```python
import numpy as np

kernel_name = "dist_rope_attn_htp_bs_b2_sq512_d1024_hq8_dh128"

def setup_inputs():
    x = np.random.randn(8, 512, 1024).astype(np.float32)
    Wq = np.random.randn(1024, 4096).astype(np.float32) * 0.02
    Wk = np.random.randn(1024, 4096).astype(np.float32) * 0.02
    Wv = np.random.randn(1024, 4096).astype(np.float32) * 0.02
    Wo = np.random.randn(4096, 1024).astype(np.float32) * 0.02
    return {"x": x, "Wq": Wq, "Wk": Wk, "Wv": Wv, "Wo": Wo}

def reference(x, Wq, Wk, Wv, Wo):
    B, Sq, Hq, Dh = 8, 512, 32, 128
    inv = 1.0 / (10000.0 ** (np.arange(0, Dh, 2) / Dh))
    pos = np.arange(Sq)[:, None] * inv[None, :]
    cos = np.repeat(np.cos(pos), 2, axis=-1).astype(np.float32)
    sin = np.repeat(np.sin(pos), 2, axis=-1).astype(np.float32)
    def rot(t):
        t2 = t.reshape(B, Sq, Hq, Dh // 2, 2)
        t_r = np.stack([-t2[..., 1], t2[..., 0]], axis=-1).reshape(B, Sq, Hq, Dh)
        return t * cos[None, :, None, :] + t_r * sin[None, :, None, :]
    Q = rot((x @ Wq).reshape(B, Sq, Hq, Dh))
    K = rot((x @ Wk).reshape(B, Sq, Hq, Dh))
    V = (x @ Wv).reshape(B, Sq, Hq, Dh)
    s = np.einsum('bihd,bjhd->bhij', Q, K).astype(np.float32) * 0.08838834764831843
    s_max = s.max(axis=-1, keepdims=True)
    w = np.exp(s - s_max)
    w = w / w.sum(axis=-1, keepdims=True)
    ctx = np.einsum('bhij,bjhd->bihd', w, V).reshape(B, Sq, Hq * Dh)
    return ctx @ Wo
```

```python
import numpy as np
import jax
import jax.numpy as jnp
from jax import lax
from jax.experimental import pallas as pl
from jax.experimental.pallas import tpu as pltpu

N_DEV = 4
BL = 2
S = 512
D = 1024
HL = 8
DH = 128
SCALE = 0.08838834764831843
LOG2E = 1.4426950408889634

_inv = 1.0 / (10000.0 ** (np.arange(0, DH, 2) / DH))
_pos = np.arange(S)[:, None] * _inv[None, :]
_cos = np.repeat(np.cos(_pos), 2, axis=-1).astype(np.float32)
_sin = np.repeat(np.sin(_pos), 2, axis=-1).astype(np.float32)
_sgn = np.where(np.arange(DH) % 2 == 0, -1.0, 1.0).astype(np.float32)[None, :]
_TAB = np.stack([
    _cos * np.float32(SCALE * LOG2E), _sin * _sgn * np.float32(SCALE * LOG2E),
    _cos, _sin * _sgn,
]).astype(np.float32)

_ORDER = (0, 4, 2, 6, 7, 5, 3, 1)
_ORDER_PACKED = sum(s << (4 * i) for i, s in enumerate(_ORDER))


def _body(x_hbm, wq_hbm, wk_hbm, wv_hbm, wo_hbm, tab_ref, out_hbm,
          xf, xg, wst, wb, ctx, psend, precv, own,
          ld_sem, ag_send, ag_recv, rs_send, rs_recv, out_sem):
    me = lax.axis_index("i")
    left = (me + N_DEV - 1) % N_DEV
    right = (me + 1) % N_DEV
    far = (me + 2) % N_DEV

    x_ld = [pltpu.make_async_copy(x_hbm.at[b], xf.at[b], ld_sem.at[b]) for b in range(BL)]
    w_ld = [pltpu.make_async_copy(w, wst.at[i], ld_sem.at[BL + i])
            for i, w in enumerate((wq_hbm, wk_hbm, wv_hbm, wo_hbm))]
    x_ld[0].start()
    x_ld[1].start()
    for c in w_ld:
        c.start()

    def ag_copy(b, k):
        dev = (right, left, far)[k]
        return pltpu.make_async_remote_copy(
            src_ref=xg.at[b], dst_ref=xg.at[2 + 2 * k + b],
            send_sem=ag_send.at[2 * k + b], recv_sem=ag_recv.at[2 * k + b],
            device_id=(dev,), device_id_type=pl.DeviceIdType.MESH)

    for b in range(BL):
        x_ld[b].wait()
        xg[b] = xf[b].astype(jnp.bfloat16)
        for k in range(3):
            ag_copy(b, k).start()
    for i in range(4):
        w_ld[i].wait()
        wb[i] = wst[i].astype(jnp.bfloat16)

    def rs_copy(k, b):
        dev = (left, right, far)[k]
        kk = (1, 0, 2)[k]
        return pltpu.make_async_remote_copy(
            src_ref=psend.at[2 * k + b], dst_ref=precv.at[2 * kk + b],
            send_sem=rs_send.at[2 * k + b], recv_sem=rs_recv.at[2 * kk + b],
            device_id=(dev,), device_id_type=pl.DeviceIdType.MESH)

    lane = lax.broadcasted_iota(jnp.int32, (S, DH), 1)
    even = (lane % 2) == 0

    def rope(t, c, s):
        sw = jnp.where(even, pltpu.roll(t, DH - 1, 1), pltpu.roll(t, 1, 1))
        return t * c + sw * s

    def finish(b):
        for k in range(3):
            rs_copy(k, b).wait_recv()
        own[b] = (own[b] + precv[b].astype(jnp.float32)
                  + precv[2 + b].astype(jnp.float32) + precv[4 + b].astype(jnp.float32))
        pltpu.make_async_copy(own.at[b], out_hbm.at[b], out_sem.at[b]).start()

    def step(i, carry):
        slot = (_ORDER_PACKED >> (4 * i)) & 7
        for s_ in range(2, 8):
            @pl.when(slot == s_)
            def _():
                ag_copy(s_ % 2, (s_ - 2) // 2).wait_recv()

        xb = xg[slot]
        for hp in range(HL // 2):
            cs = slice(hp * 2 * DH, (hp + 1) * 2 * DH)
            q2 = jnp.dot(xb, wb[0, :, cs], preferred_element_type=jnp.float32)
            k2 = jnp.dot(xb, wb[1, :, cs], preferred_element_type=jnp.float32)
            v2 = jnp.dot(xb, wb[2, :, cs], preferred_element_type=jnp.float32)
            for j in range(2):
                hs = slice(j * DH, (j + 1) * DH)
                q = rope(q2[:, hs], tab_ref[0], tab_ref[1]).astype(jnp.bfloat16)
                k = rope(k2[:, hs], tab_ref[2], tab_ref[3]).astype(jnp.bfloat16)
                v = v2[:, hs].astype(jnp.bfloat16)
                s = lax.dot_general(q, k, (((1,), (1,)), ((), ())),
                                    preferred_element_type=jnp.float32)
                m = jnp.max(s, axis=-1, keepdims=True)
                p = jnp.exp2(s - m)
                l = jnp.sum(p, axis=-1, keepdims=True)
                o = jnp.dot(p.astype(jnp.bfloat16), v, preferred_element_type=jnp.float32)
                h = hp * 2 + j
                ctx[:, h * DH:(h + 1) * DH] = (o * (1.0 / l)).astype(jnp.bfloat16)
        part = jnp.dot(ctx[...], wb[3], preferred_element_type=jnp.float32)

        @pl.when(slot < 2)
        def _():
            own[slot] = part

        @pl.when(slot >= 2)
        def _():
            psend[slot - 2] = part.astype(jnp.bfloat16)

        for s_ in range(2, 8):
            @pl.when(slot == s_)
            def _():
                rs_copy((s_ - 2) // 2, s_ % 2).start()

        @pl.when(i == 6)
        def _():
            finish(0)
        return carry

    lax.fori_loop(0, 8, step, 0)
    finish(1)
    for b in range(BL):
        pltpu.make_async_copy(own.at[b], out_hbm.at[b], out_sem.at[b]).wait()
        for k in range(3):
            ag_copy(b, k).wait_send()
            rs_copy(k, b).wait_send()


def pallas_dist_rope_attn_htp_bs_b2_sq512_d1024_hq8_dh128_kernel(x, Wq, Wk, Wv, Wo):
    any_spec = pl.BlockSpec(memory_space=pl.ANY)
    return pl.pallas_call(
        _body,
        out_shape=jax.ShapeDtypeStruct((BL, S, D), jnp.float32),
        in_specs=[any_spec] * 5 + [pl.BlockSpec(memory_space=pltpu.VMEM)],
        out_specs=any_spec,
        scratch_shapes=[
            pltpu.VMEM((BL, S, D), jnp.float32),
            pltpu.VMEM((8, S, D), jnp.bfloat16),
            pltpu.VMEM((4, D, D), jnp.float32),
            pltpu.VMEM((4, D, D), jnp.bfloat16),
            pltpu.VMEM((S, D), jnp.bfloat16),
            pltpu.VMEM((6, S, D), jnp.bfloat16),
            pltpu.VMEM((6, S, D), jnp.bfloat16),
            pltpu.VMEM((BL, S, D), jnp.float32),
            pltpu.SemaphoreType.DMA((6,)),
            pltpu.SemaphoreType.DMA((6,)),
            pltpu.SemaphoreType.DMA((6,)),
            pltpu.SemaphoreType.DMA((6,)),
            pltpu.SemaphoreType.DMA((6,)),
            pltpu.SemaphoreType.DMA((2,)),
        ],
        compiler_params=pltpu.CompilerParams(vmem_limit_bytes=100 * 1024 * 1024),
    )(x, Wq, Wk, Wv, Wo, jnp.asarray(_TAB))
```

```python
import numpy as np
import jax
import jax.numpy as jnp
from jax import lax
from jax.experimental import pallas as pl
from jax.experimental.pallas import tpu as pltpu

N_DEV = 4
BL = 2
S = 512
D = 1024
HL = 8
DH = 128
SCALE = 0.08838834764831843
LOG2E = 1.4426950408889634

_ORDER = (0, 4, 2, 6, 7, 5, 3, 1)
_ORDER_PACKED = sum(s << (4 * i) for i, s in enumerate(_ORDER))


def _body(x_hbm, wq_hbm, wk_hbm, wv_hbm, wo_hbm, out_hbm,
          xf, xg, wst, wb, tab_ref, ctx, psend, precv, own,
          ld_sem, ag_send, ag_recv, rs_send, rs_recv, out_sem):
    me = lax.axis_index("i")
    left = (me + N_DEV - 1) % N_DEV
    right = (me + 1) % N_DEV
    far = (me + 2) % N_DEV
    NP = HL // 2
    CW = 2 * DH

    def cols(hp):
        return slice(hp * CW, (hp + 1) * CW)

    x_ld = [pltpu.make_async_copy(x_hbm.at[b], xf.at[b], ld_sem.at[b]) for b in range(BL)]
    w_ld = [[pltpu.make_async_copy(w.at[:, cols(hp)], wst.at[i, :, cols(hp)],
                                   ld_sem.at[BL + i * NP + hp]) for hp in range(NP)]
            for i, w in enumerate((wq_hbm, wk_hbm, wv_hbm, wo_hbm))]
    x_ld[0].start()
    for hp in range(NP):
        for i in range(3):
            w_ld[i][hp].start()
        if hp == 0:
            x_ld[1].start()
    for hp in range(NP):
        w_ld[3][hp].start()

    def ag_copy(b, k):
        dev = (right, left, far)[k]
        return pltpu.make_async_remote_copy(
            src_ref=xg.at[b], dst_ref=xg.at[2 + 2 * k + b],
            send_sem=ag_send.at[2 * k + b], recv_sem=ag_recv.at[2 * k + b],
            device_id=(dev,), device_id_type=pl.DeviceIdType.MESH)

    def rs_copy(k, b):
        dev = (left, right, far)[k]
        kk = (1, 0, 2)[k]
        return pltpu.make_async_remote_copy(
            src_ref=psend.at[2 * k + b], dst_ref=precv.at[2 * kk + b],
            send_sem=rs_send.at[2 * k + b], recv_sem=rs_recv.at[2 * kk + b],
            device_id=(dev,), device_id_type=pl.DeviceIdType.MESH)

    lane = lax.broadcasted_iota(jnp.int32, (S, DH), 1)
    even = (lane % 2) == 0
    row = lax.broadcasted_iota(jnp.int32, (S, DH), 0).astype(jnp.float32)
    inv = jnp.exp((lane - lane % 2).astype(jnp.float32) * (-np.log(10000.0) / DH))
    ang = row * inv
    cos = jnp.cos(ang)
    sin = jnp.where(even, -jnp.sin(ang), jnp.sin(ang))
    tab_ref[0] = cos * (SCALE * LOG2E)
    tab_ref[1] = sin * (SCALE * LOG2E)
    tab_ref[2] = cos
    tab_ref[3] = sin

    def send_x(b):
        x_ld[b].wait()
        xg[b] = xf[b].astype(jnp.bfloat16)
        for k in range(3):
            ag_copy(b, k).start()

    def rope(t, c, s):
        sw = jnp.where(even, pltpu.roll(t, DH - 1, 1), pltpu.roll(t, 1, 1))
        return t * c + sw * s

    def get_w(i, hp, first):
        if first:
            w_ld[i][hp].wait()
            wb[i, :, cols(hp)] = wst[i, :, cols(hp)].astype(jnp.bfloat16)
        return wb[i, :, cols(hp)]

    def attend(slot, first=False):
        xb = xg[slot]
        for hp in range(NP):
            q2 = jnp.dot(xb, get_w(0, hp, first), preferred_element_type=jnp.float32)
            k2 = jnp.dot(xb, get_w(1, hp, first), preferred_element_type=jnp.float32)
            v2 = jnp.dot(xb, get_w(2, hp, first), preferred_element_type=jnp.float32)
            if first and hp == 0:
                send_x(1)
            for j in range(2):
                hs = slice(j * DH, (j + 1) * DH)
                q = rope(q2[:, hs], tab_ref[0], tab_ref[1]).astype(jnp.bfloat16)
                k = rope(k2[:, hs], tab_ref[2], tab_ref[3]).astype(jnp.bfloat16)
                v = v2[:, hs].astype(jnp.bfloat16)
                s = lax.dot_general(q, k, (((1,), (1,)), ((), ())),
                                    preferred_element_type=jnp.float32)
                m = jnp.max(s, axis=-1, keepdims=True)
                p = jnp.exp2(s - m)
                l = jnp.sum(p, axis=-1, keepdims=True)
                o = jnp.dot(p.astype(jnp.bfloat16), v, preferred_element_type=jnp.float32)
                h = hp * 2 + j
                ctx[:, h * DH:(h + 1) * DH] = (o * (1.0 / l)).astype(jnp.bfloat16)

    def out_copy(b, hp):
        return pltpu.make_async_copy(own.at[b, :, cols(hp)], out_hbm.at[b, :, cols(hp)],
                                     out_sem.at[b * NP + hp])

    def recv_sum(b, hp):
        c = cols(hp)
        return (precv[b, :, c].astype(jnp.float32) + precv[2 + b, :, c].astype(jnp.float32)
                + precv[4 + b, :, c].astype(jnp.float32))

    send_x(0)
    attend(0, first=True)
    for hp in range(NP):
        own[0, :, cols(hp)] = jnp.dot(ctx[...], get_w(3, hp, True),
                                      preferred_element_type=jnp.float32)

    def step(i, carry):
        slot = (_ORDER_PACKED >> (4 * i)) & 7
        for s_ in range(2, 8):
            @pl.when(slot == s_)
            def _():
                ag_copy(s_ % 2, (s_ - 2) // 2).wait_recv()
        attend(slot)
        psend[slot - 2] = jnp.dot(ctx[...], wb[3],
                                  preferred_element_type=jnp.float32).astype(jnp.bfloat16)
        for s_ in range(2, 8):
            @pl.when(slot == s_)
            def _():
                rs_copy((s_ - 2) // 2, s_ % 2).start()
        return carry

    lax.fori_loop(1, 7, step, 0)

    for k in range(3):
        rs_copy(k, 0).wait_recv()
    for hp in range(NP):
        own[0, :, cols(hp)] += recv_sum(0, hp)
        out_copy(0, hp).start()

    attend(1)
    for k in range(3):
        rs_copy(k, 1).wait_recv()
    for hp in range(NP):
        own[1, :, cols(hp)] = recv_sum(1, hp) + jnp.dot(
            ctx[...], wb[3, :, cols(hp)], preferred_element_type=jnp.float32)
        out_copy(1, hp).start()
    for b in range(BL):
        for hp in range(NP):
            out_copy(b, hp).wait()
        for k in range(3):
            ag_copy(b, k).wait_send()
            rs_copy(k, b).wait_send()


def pallas_dist_rope_attn_htp_bs_b2_sq512_d1024_hq8_dh128_kernel(x, Wq, Wk, Wv, Wo):
    any_spec = pl.BlockSpec(memory_space=pl.ANY)
    return pl.pallas_call(
        _body,
        out_shape=jax.ShapeDtypeStruct((BL, S, D), jnp.float32),
        in_specs=[any_spec] * 5,
        out_specs=any_spec,
        scratch_shapes=[
            pltpu.VMEM((BL, S, D), jnp.float32),
            pltpu.VMEM((8, S, D), jnp.bfloat16),
            pltpu.VMEM((4, D, D), jnp.float32),
            pltpu.VMEM((4, D, D), jnp.bfloat16),
            pltpu.VMEM((4, S, DH), jnp.float32),
            pltpu.VMEM((S, D), jnp.bfloat16),
            pltpu.VMEM((6, S, D), jnp.bfloat16),
            pltpu.VMEM((6, S, D), jnp.bfloat16),
            pltpu.VMEM((BL, S, D), jnp.float32),
            pltpu.SemaphoreType.DMA((18,)),
            pltpu.SemaphoreType.DMA((6,)),
            pltpu.SemaphoreType.DMA((6,)),
            pltpu.SemaphoreType.DMA((6,)),
            pltpu.SemaphoreType.DMA((6,)),
            pltpu.SemaphoreType.DMA((8,)),
        ],
        compiler_params=pltpu.CompilerParams(vmem_limit_bytes=100 * 1024 * 1024),
    )(x, Wq, Wk, Wv, Wo)
```

```python
import numpy as np
import jax
import jax.numpy as jnp
from jax import lax
from jax.experimental import pallas as pl
from jax.experimental.pallas import tpu as pltpu

N_DEV = 4
BL = 2
S = 512
D = 1024
HL = 8
DH = 128
SCALE = 0.08838834764831843
LOG2E = 1.4426950408889634

_inv = 1.0 / (10000.0 ** (np.arange(0, DH, 2) / DH))
_pos = np.arange(S)[:, None] * _inv[None, :]
_sgn = np.where(np.arange(DH) % 2 == 0, -1.0, 1.0)[None, :]
_cos = np.repeat(np.cos(_pos), 2, axis=-1)
_sin = np.repeat(np.sin(_pos), 2, axis=-1) * _sgn
_TAB = np.stack([_cos * (SCALE * LOG2E), _sin * (SCALE * LOG2E), _cos, _sin]).astype(np.float32)

_ORDER = (0, 4, 2, 6, 7, 5, 3, 1)
_ORDER_PACKED = sum(s << (4 * i) for i, s in enumerate(_ORDER))


def _body(x_hbm, wq_hbm, wk_hbm, wv_hbm, wo_hbm, tab_hbm, own,
          xf, xg, wst, wb, tab_ref, ctx, psend, precv,
          ld_sem, ag_send, ag_recv, rs_send, rs_recv):
    me = lax.axis_index("i")
    left = (me + N_DEV - 1) % N_DEV
    right = (me + 1) % N_DEV
    far = (me + 2) % N_DEV
    NP = HL // 2
    CW = 2 * DH
    KS = (NP - 1) * CW

    def cols(hp):
        return slice(hp * CW, (hp + 1) * CW)

    x_ld = [pltpu.make_async_copy(x_hbm.at[b], xf.at[b], ld_sem.at[b]) for b in range(BL)]
    w_ld = [[pltpu.make_async_copy(w.at[:, cols(hp)], wst.at[i, :, cols(hp)],
                                   ld_sem.at[BL + i * NP + hp]) for hp in range(NP)]
            for i, w in enumerate((wq_hbm, wk_hbm, wv_hbm, wo_hbm))]
    tab_ld = pltpu.make_async_copy(tab_hbm, tab_ref, ld_sem.at[18])

    def ag_copy(b, k):
        dev = (right, left, far)[k]
        return pltpu.make_async_remote_copy(
            src_ref=xg.at[b], dst_ref=xg.at[2 + 2 * k + b],
            send_sem=ag_send.at[2 * k + b], recv_sem=ag_recv.at[2 * k + b],
            device_id=(dev,), device_id_type=pl.DeviceIdType.MESH)

    def rs_copy(k, b):
        dev = (left, right, far)[k]
        kk = (1, 0, 2)[k]
        return pltpu.make_async_remote_copy(
            src_ref=psend.at[2 * k + b], dst_ref=precv.at[2 * kk + b],
            send_sem=rs_send.at[2 * k + b], recv_sem=rs_recv.at[2 * kk + b],
            device_id=(dev,), device_id_type=pl.DeviceIdType.MESH)

    lane = lax.broadcasted_iota(jnp.int32, (S, DH), 1)
    even = (lane % 2) == 0
    def send_x(b):
        x_ld[b].wait()
        xg[b] = xf[b].astype(jnp.bfloat16)
        if b == 0:
            pl.semaphore_wait(pltpu.get_barrier_semaphore(), 3)
        for k in range(3 if b else 2):
            ag_copy(b, k).start()

    def rope(t, c, s):
        sw = jnp.where(even, pltpu.roll(t, DH - 1, 1), pltpu.roll(t, 1, 1))
        return t * c + sw * s

    def get_w(i, hp, first):
        if first:
            w_ld[i][hp].wait()
            wb[i, :, cols(hp)] = wst[i, :, cols(hp)].astype(jnp.bfloat16)
        return wb[i, :, cols(hp)]

    def attend(slot, first=False, c=0):
        xb = xg[slot]
        for hp in range(NP):
            if first:
                if hp == 0:
                    for h2 in range(1, NP):
                        for i in range(3):
                            w_ld[i][h2].start()
                if hp == NP - 1:
                    x_ld[1].start()
                    for cp in w_ld[3]:
                        cp.start()
            if first and hp > 0:
                for i in range(3):
                    get_w(i, hp, True)
            q2 = jnp.dot(xb, get_w(0, hp, first and hp == 0), preferred_element_type=jnp.float32)
            k2 = jnp.dot(xb, get_w(1, hp, first and hp == 0), preferred_element_type=jnp.float32)
            v2 = jnp.dot(xb, get_w(2, hp, first and hp == 0), preferred_element_type=jnp.float32)
            if first and hp == 0:
                tab_ld.wait()
            if first and hp == 1:
                ag_copy(0, 2).start()
            if hp == NP - 1 and not first:
                acc = jnp.dot(ctx[0, :, :KS], wb[3, :KS, :], preferred_element_type=jnp.float32)
            for j in range(2):
                hs = slice(j * DH, (j + 1) * DH)
                q = rope(q2[:, hs], tab_ref[0], tab_ref[1]).astype(jnp.bfloat16)
                k = rope(k2[:, hs], tab_ref[2], tab_ref[3]).astype(jnp.bfloat16)
                v = v2[:, hs].astype(jnp.bfloat16)
                s = lax.dot_general(q, k, (((1,), (1,)), ((), ())),
                                    preferred_element_type=jnp.float32)
                m = jnp.max(s, axis=-1, keepdims=True)
                p = jnp.exp2(s - m)
                l = jnp.sum(p, axis=-1, keepdims=True)
                o = jnp.dot(p.astype(jnp.bfloat16), v, preferred_element_type=jnp.float32)
                h = hp * 2 + j
                ctx[c, :, h * DH:(h + 1) * DH] = (o * (1.0 / l)).astype(jnp.bfloat16)

        if not first:
            return acc + jnp.dot(ctx[0, :, KS:], wb[3, KS:, :],
                                 preferred_element_type=jnp.float32)

    def recv_sum(b, hp):
        c = cols(hp)
        return (precv[b, :, c].astype(jnp.float32) + precv[2 + b, :, c].astype(jnp.float32)
                + precv[4 + b, :, c].astype(jnp.float32))

    def first_step():
        bar = pltpu.get_barrier_semaphore()
        for dev in (left, right, far):
            pl.semaphore_signal(bar, inc=1, device_id=(dev,),
                                device_id_type=pl.DeviceIdType.MESH)
        x_ld[0].start()
        for i in range(3):
            w_ld[i][0].start()
        tab_ld.start()
        send_x(0)
        attend(0, first=True, c=1)

    first_step()

    @pl.loop(1, 7)
    def _(step):
        slot = (_ORDER_PACKED >> (4 * step)) & 7

        @pl.when(step == 1)
        def _():
            send_x(1)
            for hp in range(NP):
                get_w(3, hp, True)

        for s_ in range(2, 8):
            @pl.when(slot == s_)
            def _():
                ag_copy(s_ % 2, (s_ - 2) // 2).wait_recv()
        part = attend(slot)
        psend[slot - 2] = part.astype(jnp.bfloat16)
        k = (slot - 2) // 2
        b = slot % 2
        kk = jnp.where(k == 2, 2, 1 - k)
        dev = jnp.where(k == 0, left, jnp.where(k == 1, right, far))
        pltpu.make_async_remote_copy(
            src_ref=psend.at[slot - 2], dst_ref=precv.at[2 * kk + b],
            send_sem=rs_send.at[slot - 2], recv_sem=rs_recv.at[2 * kk + b],
            device_id=(dev,), device_id_type=pl.DeviceIdType.MESH).start()

    for k in range(3):
        rs_copy(k, 0).wait_recv()
    for hp in range(NP):
        own[0, :, cols(hp)] = recv_sum(0, hp) + jnp.dot(
            ctx[1], wb[3, :, cols(hp)], preferred_element_type=jnp.float32)

    own[1] = attend(1)
    for k in range(3):
        rs_copy(k, 1).wait_recv()
    for hp in range(NP):
        own[1, :, cols(hp)] += recv_sum(1, hp)
    for b in range(BL):
        for k in range(3):
            ag_copy(b, k).wait_send()
            rs_copy(k, b).wait_send()


def pallas_dist_rope_attn_htp_bs_b2_sq512_d1024_hq8_dh128_kernel(x, Wq, Wk, Wv, Wo):
    any_spec = pl.BlockSpec(memory_space=pl.ANY)
    return pl.pallas_call(
        _body,
        out_shape=jax.ShapeDtypeStruct((BL, S, D), jnp.float32),
        in_specs=[any_spec] * 6,
        out_specs=pl.BlockSpec(memory_space=pltpu.VMEM),
        scratch_shapes=[
            pltpu.VMEM((BL, S, D), jnp.float32),
            pltpu.VMEM((8, S, D), jnp.bfloat16),
            pltpu.VMEM((4, D, D), jnp.float32),
            pltpu.VMEM((4, D, D), jnp.bfloat16),
            pltpu.VMEM((4, S, DH), jnp.float32),
            pltpu.VMEM((2, S, D), jnp.bfloat16),
            pltpu.VMEM((6, S, D), jnp.bfloat16),
            pltpu.VMEM((6, S, D), jnp.bfloat16),
            pltpu.SemaphoreType.DMA((19,)),
            pltpu.SemaphoreType.DMA((6,)),
            pltpu.SemaphoreType.DMA((6,)),
            pltpu.SemaphoreType.DMA((6,)),
            pltpu.SemaphoreType.DMA((6,)),
        ],
        compiler_params=pltpu.CompilerParams(collective_id=0, vmem_limit_bytes=100 * 1024 * 1024),
    )(x, Wq, Wk, Wv, Wo, jnp.asarray(_TAB))
```
